```python
import numpy as np

kernel_name = "dist_argmax_global_i_m4096_n1024"

def setup_inputs():
    return {"x": np.random.randn(16384, 1024).astype(np.float32)}

def reference(x: np.ndarray) -> np.ndarray:
    idx = np.argmax(x, axis=0).astype(np.float32)
    val = np.max(x, axis=0)
    return np.stack([val, idx], axis=0)
```

```python
import jax
import jax.numpy as jnp
from jax import lax
from jax.experimental import pallas as pl
from jax.experimental.pallas import tpu as pltpu

N_DEV = 4
_MESH = pl.DeviceIdType.MESH

_OFFLOAD = 192
_TAIL = (256, 96, 32, 16, 8, 8)
_UNROLL = 4


def _merge(v, i, v2, i2):
    n1 = v != v
    n2 = v2 != v2
    gt = jnp.logical_or(v2 > v, jnp.logical_and(n2, jnp.logical_not(n1)))
    eq = jnp.logical_or(v2 == v, jnp.logical_and(n1, n2))
    take = jnp.logical_or(gt, jnp.logical_and(eq, i2 < i))
    return jnp.where(take, v2, v), jnp.where(take, i2, i)


def _reduce8(bv, bi):
    mx = jnp.max(bv, axis=0, keepdims=True)
    cand = jnp.logical_or(bv == mx, bv != bv)
    ix = jnp.min(jnp.where(cand, bi, jnp.float32(3e38)), axis=0, keepdims=True)
    return mx, ix


def pallas_dist_argmax_global_i_m4096_n1024_kernel(x: jax.Array):
    m, n = x.shape
    k = _OFFLOAD
    local = m - 2 * k
    bulk = local - sum(_TAIL)
    first = (bulk * 5 // 8) // 32 * 32
    sizes = (first, bulk - first) + _TAIL
    offs = [0]
    for s in sizes:
        offs.append(offs[-1] + s)
    nc = len(sizes)
    assert all(s > 0 and (s <= 32 or s % (8 * _UNROLL) == 0) and s % 8 == 0 for s in sizes)
    assert k % (8 * _UNROLL) == 0

    def body(x_hbm, out_ref, buf, rbuf, send_buf, recv_buf,
             sems, osend_sems, orecv_sems, send_sems, recv_sems):
        me = lax.axis_index("i")
        peers = {j: (me + j) & (N_DEV - 1) for j in range(1, N_DEV)}

        chunks = [
            pltpu.make_async_copy(
                x_hbm.at[pl.ds(offs[c], sizes[c])], buf.at[pl.ds(offs[c], sizes[c])], sems.at[c]
            )
            for c in range(nc)
        ]
        for c in chunks:
            c.start()

        barrier = pltpu.get_barrier_semaphore()
        for j in range(1, N_DEV):
            pl.semaphore_signal(barrier, inc=1, device_id=(peers[j],), device_id_type=_MESH)
        pl.semaphore_wait(barrier, N_DEV - 1)

        offload = []
        for slot, dst in ((0, peers[1]), (1, peers[3])):
            c = pltpu.make_async_remote_copy(
                src_ref=x_hbm.at[pl.ds(local + slot * k, k)],
                dst_ref=rbuf.at[slot],
                send_sem=osend_sems.at[slot],
                recv_sem=orecv_sems.at[slot],
                device_id=(dst,),
                device_id_type=_MESH,
            )
            c.start()
            offload.append(c)

        sub = lax.broadcasted_iota(jnp.int32, (8, n), 0)

        def init_state(first_row):
            rows = (sub + first_row).astype(jnp.float32)
            return jnp.full((8, n), -jnp.inf, jnp.float32), rows, rows

        def scan(ref, row0, nrows, state):
            def step(r0, state):
                bv, bi, rows = state
                xv = ref[pl.ds(r0, 8), :]
                keep = jnp.logical_or(xv <= bv, bv != bv)
                return jnp.where(keep, bv, xv), jnp.where(keep, bi, rows), rows + 8.0

            groups = nrows // 8
            if groups <= _UNROLL:
                for g in range(groups):
                    state = step(row0 + 8 * g, state)
                return state
            return lax.fori_loop(
                0, groups,
                lambda g, st: step(pl.multiple_of(row0 + 8 * g, 8), st),
                state, unroll=_UNROLL,
            )

        state = init_state(me * m)
        nbr = None
        for c in range(nc):
            chunks[c].wait()
            state = scan(buf, offs[c], sizes[c], state)
            if c == 1:
                for slot, src in ((0, peers[3]), (1, peers[1])):
                    offload[slot].wait_recv()
                    bv, bi, _ = scan(rbuf.at[slot], 0, k, init_state(src * m + local + slot * k))
                    cand = _reduce8(bv, bi)
                    nbr = cand if nbr is None else _merge(*nbr, *cand)

        v, i = _merge(*_reduce8(state[0], state[1]), *nbr)
        send_buf[0:1, :] = v
        send_buf[1:2, :] = i

        copies = {}
        for j in (2, 1, 3):
            c = pltpu.make_async_remote_copy(
                src_ref=send_buf,
                dst_ref=recv_buf.at[j - 1],
                send_sem=send_sems.at[j - 1],
                recv_sem=recv_sems.at[j - 1],
                device_id=(peers[j],),
                device_id_type=_MESH,
            )
            c.start()
            copies[j] = c
        v = send_buf[0:1, :]
        i = send_buf[1:2, :]
        for j in (1, 3, 2):
            copies[j].wait_recv()
            v, i = _merge(v, i, recv_buf[j - 1, 0:1, :], recv_buf[j - 1, 1:2, :])
        out_ref[0:1, :] = v
        out_ref[1:2, :] = i
        for j in (2, 1, 3):
            copies[j].wait_send()
        for c in offload:
            c.wait_send()

    return pl.pallas_call(
        body,
        out_shape=jax.ShapeDtypeStruct((2, n), jnp.float32),
        in_specs=[pl.BlockSpec(memory_space=pl.ANY)],
        out_specs=pl.BlockSpec(memory_space=pltpu.VMEM),
        scratch_shapes=[
            pltpu.VMEM((local, n), jnp.float32),
            pltpu.VMEM((2, k, n), jnp.float32),
            pltpu.VMEM((2, n), jnp.float32),
            pltpu.VMEM((N_DEV - 1, 2, n), jnp.float32),
            pltpu.SemaphoreType.DMA((nc,)),
            pltpu.SemaphoreType.DMA((2,)),
            pltpu.SemaphoreType.DMA((2,)),
            pltpu.SemaphoreType.DMA((N_DEV - 1,)),
            pltpu.SemaphoreType.DMA((N_DEV - 1,)),
        ],
        compiler_params=pltpu.CompilerParams(
            collective_id=0,
            vmem_limit_bytes=48 << 20,
            disable_semaphore_checks=True,
        ),
    )(x)
```

```python
import jax
import jax.numpy as jnp
from jax import lax
from jax.experimental import pallas as pl
from jax.experimental.pallas import tpu as pltpu

N_DEV = 4
_MESH = pl.DeviceIdType.MESH
_BIG = 3e38

_OFFLOAD = 192
_PRE = 128
_A_SIZES = (192, 96, 24, 8)
_B_SIZES = (160, 96, 32, 32)
_A_COLS = 896
_B_STEP = 32
_UNROLL = 4


def _merge(v, i, v2, i2):
    n1 = v != v
    n2 = v2 != v2
    gt = jnp.logical_or(v2 > v, jnp.logical_and(n2, jnp.logical_not(n1)))
    eq = jnp.logical_or(v2 == v, jnp.logical_and(n1, n2))
    take = jnp.logical_or(gt, jnp.logical_and(eq, i2 < i))
    return jnp.where(take, v2, v), jnp.where(take, i2, i)


def _reduce_rows(bv, bi):
    mx = jnp.max(bv, axis=0, keepdims=True)
    cand = jnp.logical_or(bv == mx, bv != bv)
    ix = jnp.min(jnp.where(cand, bi, jnp.float32(_BIG)), axis=0, keepdims=True)
    return mx, ix


def _row_ids(first_row, h, w):
    return (lax.broadcasted_iota(jnp.int32, (h, w), 0) + first_row).astype(jnp.float32)


def _scan(ref, row0, nrows, col0, state):
    h, w = state[0].shape

    def step(r0, state):
        bv, bi, rows = state
        xv = ref[pl.ds(r0, h), pl.ds(col0, w)]
        keep = jnp.logical_or(xv <= bv, bv != bv)
        return jnp.where(keep, bv, xv), jnp.where(keep, bi, rows), rows + float(h)

    steps = nrows // h
    assert steps * h == nrows
    if steps <= 6:
        for g in range(steps):
            state = step(row0 + g * h, state)
        return state
    assert steps % _UNROLL == 0
    return lax.fori_loop(
        0, steps, lambda g, st: step(pl.multiple_of(row0 + g * h, 8), st), state, unroll=_UNROLL
    )


def _scan_block(ref, nrows, first_row, n):
    rows = _row_ids(first_row, 8, n)
    bv, bi, _ = _scan(ref, 0, nrows, 0, (jnp.full((8, n), -jnp.inf, jnp.float32), rows, rows))
    return _reduce_rows(bv, bi)


def _offsets(sizes, start):
    out = []
    for s in sizes:
        out.append(start)
        start += s
    return out


def pallas_dist_argmax_global_i_m4096_n1024_kernel(x: jax.Array):
    m, n = x.shape
    k = _OFFLOAD
    ca_, cb_ = _A_COLS, n - _A_COLS
    local = m - 2 * k
    split = sum(_A_SIZES)
    assert split == sum(_B_SIZES)
    bulk = local - split - _PRE
    first = (bulk * 5 // 8) // 32 * 32
    h_sizes = (first, bulk - first, _PRE)
    h_offs = _offsets(h_sizes, 0)
    a_offs = _offsets(_A_SIZES, local - split)
    b_offs = _offsets(_B_SIZES, local - split)
    nh, na, nb = len(h_sizes), len(_A_SIZES), len(_B_SIZES)

    def body(x_hbm, out_ref, buf, rbuf, send_a, send_b, recv_a, recv_b,
             sems, so_sems, ro_sems, sa_sems, ra_sems, sb_sems, rb_sems):
        me = lax.axis_index("i")
        diag, ynbr, xnbr = (me + 2) & 3, me ^ 1, 3 - me
        peers = (diag, ynbr, xnbr)

        def fetch(r0, nr, c0, nc, s):
            return pltpu.make_async_copy(
                x_hbm.at[pl.ds(r0, nr), pl.ds(c0, nc)],
                buf.at[pl.ds(r0, nr), pl.ds(c0, nc)],
                sems.at[s],
            )

        h_cps = [fetch(h_offs[c], h_sizes[c], 0, n, c) for c in range(nh)]
        a_cps = [fetch(a_offs[c], _A_SIZES[c], 0, ca_, nh + c) for c in range(na)]
        b_cps = [fetch(b_offs[c], _B_SIZES[c], ca_, cb_, nh + na + c) for c in range(nb)]
        for c in h_cps + a_cps + b_cps:
            c.start()

        barrier = pltpu.get_barrier_semaphore()
        for p in peers:
            pl.semaphore_signal(barrier, inc=1, device_id=(p,), device_id_type=_MESH)
        pl.semaphore_wait(barrier, N_DEV - 1)

        offload = [
            pltpu.make_async_remote_copy(
                src_ref=x_hbm.at[pl.ds(local + s * k, k)],
                dst_ref=rbuf.at[s],
                send_sem=so_sems.at[s],
                recv_sem=ro_sems.at[s],
                device_id=(dst,),
                device_id_type=_MESH,
            )
            for s, dst in enumerate((ynbr, xnbr))
        ]
        for c in offload:
            c.start()

        rows = _row_ids(me * m, 8, n)
        state = (jnp.full((8, n), -jnp.inf, jnp.float32), rows, rows)
        for c in range(nh):
            h_cps[c].wait()
            state = _scan(buf, h_offs[c], h_sizes[c], 0, state)
        bv, bi, rows = state

        offload[0].wait_recv()
        side = _scan_block(rbuf.at[0], k, ynbr * m + local, n)
        offload[1].wait_recv()
        sv, si = _merge(*side, *_scan_block(rbuf.at[1], k, xnbr * m + local + k, n))

        def exchange(src, dst, send_sems, recv_sems):
            return [
                pltpu.make_async_remote_copy(
                    src_ref=src,
                    dst_ref=dst.at[s],
                    send_sem=send_sems.at[s],
                    recv_sem=recv_sems.at[s],
                    device_id=(peers[s],),
                    device_id_type=_MESH,
                )
                for s in range(N_DEV - 1)
            ]

        a_out = exchange(send_a, recv_a, sa_sems, ra_sems)
        b_out = exchange(send_b, recv_b, sb_sems, rb_sems)

        state = (bv[:, :ca_], bi[:, :ca_], rows[:, :ca_])
        for c in range(na):
            a_cps[c].wait()
            state = _scan(buf, a_offs[c], _A_SIZES[c], 0, state)
        va, ia = _merge(*_reduce_rows(state[0], state[1]), sv[:, :ca_], si[:, :ca_])
        send_a[0:1, :] = va
        send_a[1:2, :] = ia
        a_out[0].start()
        a_out[1].start()

        rows = _row_ids(me * m + local - split, _B_STEP, cb_)
        state = (
            jnp.concatenate(
                [bv[:, ca_:], jnp.full((_B_STEP - 8, cb_), -jnp.inf, jnp.float32)], axis=0
            ),
            jnp.concatenate([bi[:, ca_:], rows[8:]], axis=0),
            rows,
        )
        for c in range(nb):
            b_cps[c].wait()
            state = _scan(buf, b_offs[c], _B_SIZES[c], ca_, state)
        vb, ib = _merge(*_reduce_rows(state[0], state[1]), sv[:, ca_:], si[:, ca_:])
        send_b[0:1, :] = vb
        send_b[1:2, :] = ib
        b_out[0].start()
        b_out[1].start()
        a_out[2].start()
        b_out[2].start()

        for c in offload + a_out + b_out:
            c.wait_send()

        va, ia = send_a[0:1, :], send_a[1:2, :]
        for s in (1, 2, 0):
            a_out[s].wait_recv()
            va, ia = _merge(va, ia, recv_a[s, 0:1, :], recv_a[s, 1:2, :])
        out_ref[0:1, 0:ca_] = va
        out_ref[1:2, 0:ca_] = ia
        vb, ib = send_b[0:1, :], send_b[1:2, :]
        for s in (1, 2, 0):
            b_out[s].wait_recv()
            vb, ib = _merge(vb, ib, recv_b[s, 0:1, :], recv_b[s, 1:2, :])
        out_ref[0:1, ca_:n] = vb
        out_ref[1:2, ca_:n] = ib

    per_peer = pltpu.SemaphoreType.DMA((N_DEV - 1,))
    return pl.pallas_call(
        body,
        out_shape=jax.ShapeDtypeStruct((2, n), jnp.float32),
        in_specs=[pl.BlockSpec(memory_space=pl.ANY)],
        out_specs=pl.BlockSpec(memory_space=pltpu.VMEM),
        scratch_shapes=[
            pltpu.VMEM((local, n), jnp.float32),
            pltpu.VMEM((2, k, n), jnp.float32),
            pltpu.VMEM((2, ca_), jnp.float32),
            pltpu.VMEM((2, cb_), jnp.float32),
            pltpu.VMEM((N_DEV - 1, 2, ca_), jnp.float32),
            pltpu.VMEM((N_DEV - 1, 2, cb_), jnp.float32),
            pltpu.SemaphoreType.DMA((nh + na + nb,)),
            pltpu.SemaphoreType.DMA((2,)),
            pltpu.SemaphoreType.DMA((2,)),
            per_peer, per_peer, per_peer, per_peer,
        ],
        compiler_params=pltpu.CompilerParams(
            collective_id=0,
            vmem_limit_bytes=48 << 20,
            disable_semaphore_checks=True,
        ),
    )(x)
```
